```python
import numpy as np

kernel_name = "dist_mean_ax0_shard0_i_m1024_n512"

def setup_inputs():
    return {"x": np.random.randn(4096, 512).astype(np.float32)}

def reference(x: np.ndarray) -> np.ndarray:
    return np.mean(x, axis=0, keepdims=True)
```

```python
import jax
import jax.numpy as jnp
from jax import lax
from jax.experimental import pallas as pl
from jax.experimental.pallas import tpu as pltpu

N_DEV = 4
N_CHUNKS = 8


def pallas_dist_mean_ax0_shard0_i_m1024_n512_kernel(
    x: jax.Array,
):
    m, n = x.shape
    rows = m // N_CHUNKS
    inv_total = 1.0 / (m * N_DEV)

    def body(x_hbm, out_ref, buf, comm, load_sems, send_sems, recv_sems):
        my = lax.axis_index("i")

        loads = []
        for c in range(N_CHUNKS):
            cp = pltpu.make_async_copy(
                x_hbm.at[pl.ds(c * rows, rows), :],
                buf.at[pl.ds(c * rows, rows), :],
                load_sems.at[c],
            )
            cp.start()
            loads.append(cp)

        barrier = pltpu.get_barrier_semaphore()
        for k in range(1, N_DEV):
            pl.semaphore_signal(
                barrier,
                inc=1,
                device_id=((my + k) % N_DEV,),
                device_id_type=pl.DeviceIdType.MESH,
            )

        acc = jnp.zeros((8, n), jnp.float32)
        for c in range(N_CHUNKS):
            loads[c].wait()
            blk = buf[pl.ds(c * rows, rows), :]
            acc = acc + jnp.sum(blk.reshape(rows // 8, 8, n), axis=0)
        comm[0] = jnp.sum(acc, axis=0, keepdims=True)

        pl.semaphore_wait(barrier, N_DEV - 1)

        rdmas = []
        for k in range(1, N_DEV):
            r = pltpu.make_async_remote_copy(
                src_ref=comm.at[0],
                dst_ref=comm.at[k],
                send_sem=send_sems.at[k - 1],
                recv_sem=recv_sems.at[k - 1],
                device_id=((my + k) % N_DEV,),
                device_id_type=pl.DeviceIdType.MESH,
            )
            r.start()
            rdmas.append(r)
        for r in rdmas:
            r.wait_recv()
        total = (comm[0] + comm[1]) + (comm[2] + comm[3])
        out_ref[...] = total * inv_total
        for r in rdmas:
            r.wait_send()

    return pl.pallas_call(
        body,
        out_shape=jax.ShapeDtypeStruct((1, n), jnp.float32),
        in_specs=[pl.BlockSpec(memory_space=pl.ANY)],
        out_specs=pl.BlockSpec(memory_space=pltpu.VMEM),
        scratch_shapes=[
            pltpu.VMEM((m, n), jnp.float32),
            pltpu.VMEM((N_DEV, 1, n), jnp.float32),
            pltpu.SemaphoreType.DMA((N_CHUNKS,)),
            pltpu.SemaphoreType.DMA((N_DEV - 1,)),
            pltpu.SemaphoreType.DMA((N_DEV - 1,)),
        ],
        compiler_params=pltpu.CompilerParams(collective_id=0),
    )(x)
```

```python
import jax
import jax.numpy as jnp
from jax import lax
from jax.experimental import pallas as pl
from jax.experimental.pallas import tpu as pltpu

N_DEV = 4
LATE = 2
RAW_ROWS = 40
TAIL = (96, 24, 8)
SUBLANES = 8
LANES = 128


def _compiler_params():
    kwargs = dict(collective_id=0, disable_bounds_checks=True)
    try:
        return pltpu.CompilerParams(disable_semaphore_checks=True, **kwargs)
    except TypeError:
        return pltpu.CompilerParams(**kwargs)


def pallas_dist_mean_ax0_shard0_i_m1024_n512_kernel(
    x: jax.Array,
):
    m, n = x.shape
    n_blk = n // LANES
    assert n_blk == 4 and n % LANES == 0 and m % SUBLANES == 0

    raw_total = 2 * RAW_ROWS
    x_off = m - raw_total
    sizes = (x_off - sum(TAIL),) + TAIL
    offs = [0]
    for s in sizes:
        offs.append(offs[-1] + s)
    n_chunks = len(sizes)
    scale = 1.0 / (m * N_DEV)
    send_order = (2, 1, 3)
    recv_order = (1, 3, 2)

    def body(
        x_hbm,
        out_ref,
        buf,
        raw,
        ext,
        comm,
        load_sems,
        extra_sem,
        raw_send_sems,
        raw_recv_sem,
        send_sems,
        recv_sems,
    ):
        def local_load(off, rows, sem):
            return pltpu.make_async_copy(
                x_hbm.at[pl.ds(off, rows), :], buf.at[pl.ds(off, rows), :], sem
            )

        loads = [
            local_load(offs[c], sizes[c], load_sems.at[c]) for c in range(n_chunks)
        ]
        loads[0].start()

        my = lax.axis_index("i")
        is_late = my == LATE
        not_late = my != LATE
        is_helper = lax.rem(my, 2) != (LATE % 2)

        @pl.when(not_late)
        def _():
            local_load(x_off, raw_total, extra_sem).start()

        for c in range(1, n_chunks):
            loads[c].start()

        peers = {k: lax.rem(my + k, N_DEV) for k in (1, 2, 3)}
        barrier = pltpu.get_barrier_semaphore()
        for k in send_order:
            pl.semaphore_signal(
                barrier,
                inc=1,
                device_id=(peers[k],),
                device_id_type=pl.DeviceIdType.MESH,
            )
        ext[...] = jnp.zeros(ext.shape, ext.dtype)
        pl.semaphore_wait(barrier, N_DEV - 1)

        def raw_copy(j):
            return pltpu.make_async_remote_copy(
                src_ref=x_hbm.at[pl.ds(x_off + j * RAW_ROWS, RAW_ROWS), :],
                dst_ref=raw,
                send_sem=raw_send_sems.at[j],
                recv_sem=raw_recv_sem,
                device_id=((LATE + 1 + 2 * j) % N_DEV,),
                device_id_type=pl.DeviceIdType.MESH,
            )

        @pl.when(is_late)
        def _():
            for j in range(2):
                raw_copy(j).start()

        def colsum8(ref, off, rows):
            blk = ref[pl.ds(off, rows), :]
            if rows == SUBLANES:
                return blk
            return jnp.sum(blk.reshape(rows // SUBLANES, SUBLANES, n), axis=0)

        sub = lax.broadcasted_iota(jnp.int32, (SUBLANES, LANES), 0)
        even1 = (sub & 1) == 0
        even2 = (sub & 2) == 0

        def merge(a, b, mask, k):
            t = jnp.where(mask, a, b)
            u = jnp.where(mask, b, a)
            return t + pltpu.roll(u, SUBLANES - k, 0)

        def fold(v):
            a, b, c, d = [v[:, j * LANES : (j + 1) * LANES] for j in range(n_blk)]
            return merge(merge(a, b, even1, 1), merge(c, d, even1, 1), even2, 2)

        loads[0].wait()
        acc = colsum8(buf, offs[0], sizes[0])

        @pl.when(not_late)
        def _():
            local_load(x_off, raw_total, extra_sem).wait()
            ext[...] = colsum8(buf, x_off, raw_total)

        @pl.when(is_helper)
        def _():
            raw_copy(0).wait_recv()
            ext[...] += colsum8(raw, 0, RAW_ROWS)

        acc = acc + ext[...]
        for c in range(1, n_chunks - 1):
            loads[c].wait()
            acc = acc + colsum8(buf, offs[c], sizes[c])
        e0 = fold(acc)
        f0 = e0 + pltpu.roll(e0, 4, 0)

        loads[n_chunks - 1].wait()
        e = fold(colsum8(buf, offs[n_chunks - 1], sizes[n_chunks - 1]))
        part = (((e + f0) + pltpu.roll(e, 4, 0)) * scale)[0:n_blk, :]
        comm[0] = part.astype(comm.dtype)

        sends = {}
        for k in send_order:
            sends[k] = pltpu.make_async_remote_copy(
                src_ref=comm.at[0],
                dst_ref=comm.at[k],
                send_sem=send_sems.at[k - 1],
                recv_sem=recv_sems.at[k - 1],
                device_id=(peers[k],),
                device_id_type=pl.DeviceIdType.MESH,
            )
            sends[k].start()

        @pl.when(is_late)
        def _():
            for j in range(2):
                raw_copy(j).wait_send()

        for k in send_order:
            sends[k].wait_send()

        total = part
        for k in recv_order:
            sends[k].wait_recv()
            total = total + comm[k].astype(jnp.float32)
        out_ref[...] = total

    out = pl.pallas_call(
        body,
        out_shape=jax.ShapeDtypeStruct((n_blk, LANES), jnp.float32),
        in_specs=[pl.BlockSpec(memory_space=pl.ANY)],
        out_specs=pl.BlockSpec(memory_space=pltpu.VMEM),
        scratch_shapes=[
            pltpu.VMEM((m, n), jnp.float32),
            pltpu.VMEM((RAW_ROWS, n), jnp.float32),
            pltpu.VMEM((SUBLANES, n), jnp.float32),
            pltpu.VMEM((N_DEV, n_blk, LANES), jnp.bfloat16),
            pltpu.SemaphoreType.DMA((n_chunks,)),
            pltpu.SemaphoreType.DMA,
            pltpu.SemaphoreType.DMA((2,)),
            pltpu.SemaphoreType.DMA,
            pltpu.SemaphoreType.DMA((N_DEV - 1,)),
            pltpu.SemaphoreType.DMA((N_DEV - 1,)),
        ],
        compiler_params=_compiler_params(),
    )(x)
    return out.reshape(1, n)
```
